```python
import numpy as np

kernel_name = "dist_moe_cap_ep_outshard_n2048_d512_e8_h1024"

def setup_inputs():
    x = np.random.randn(2048, 512).astype(np.float32)
    router_W = np.random.randn(512, 32).astype(np.float32) * 0.1
    scores64 = x.astype(np.float64) @ router_W.astype(np.float64)
    route_idx = np.argsort(-scores64, axis=-1)[:, :1].astype(np.int32)
    expert_W = np.random.randn(32, 512, 1024).astype(np.float32) * 0.02
    return {"x": x, "router_W": router_W, "route_idx": route_idx, "expert_W": expert_W}

def reference(x, router_W, route_idx, expert_W):
    counts = np.zeros(32, dtype=np.int64)
    out = np.zeros((2048, 1024), dtype=np.float32)
    for i in range(2048):
        e = int(route_idx[i, 0])
        if counts[e] < 51:
            out[i] = x[i] @ expert_W[e]
            counts[e] += 1
    return out
```

```python
import contextlib

import jax
import jax.numpy as jnp
from jax import lax
from jax.experimental import pallas as pl
from jax.experimental.pallas import tpu as pltpu

N_TOK = 2048
D_IN = 512
D_OUT = 1024
N_DEV = 4
E_LOC = 8
N_EXP = N_DEV * E_LOC
CAP = 51
SLOTS = 64
CHUNK = 8
N_CHUNK = 7
ROWS = N_CHUNK * CHUNK
PIECES = (2, 3, 4, N_CHUNK)
TOK_PER_DEV = N_TOK // N_DEV
TB = 128
N_TB = N_TOK // TB
HALF = D_OUT // 2
BND0 = SLOTS
UNROLL = 4

_PROFILE = False


def _scope(name):
    return jax.named_scope(name) if _PROFILE else contextlib.nullcontext()


def _kernel_body(idx_ref, x_hbm, w_hbm, out_ref,
                 wbuf, xg, ysend, stage, tbl_v, tbl_s,
                 w_sems, g_sems, tbl_sem, send_sem, recv_sems):
    me = lax.axis_index("i")

    def w_copy(j):
        return pltpu.make_async_copy(w_hbm.at[j], wbuf.at[j], w_sems.at[j])

    w_copy(0).start()

    barrier_sem = pltpu.get_barrier_semaphore()
    for k in range(1, N_DEV):
        pl.semaphore_signal(
            barrier_sem, inc=1, device_id=((me + k) % N_DEV,),
            device_id_type=pl.DeviceIdType.MESH)

    eidx = idx_ref[...]
    iota_e = lax.broadcasted_iota(jnp.int32, (N_EXP, TB), 0)
    lane_e = lax.broadcasted_iota(jnp.int32, (N_EXP, TB), 1)
    sub_t = lax.broadcasted_iota(jnp.int32, (TB, TB), 0)
    lane_t = lax.broadcasted_iota(jnp.int32, (TB, TB), 1)
    upper = jnp.where(sub_t < lane_t, 1.0, 0.0).astype(jnp.bfloat16)
    onehot = [jnp.where(iota_e == eidx[b:b + 1, :], 1.0, 0.0)
              for b in range(N_TB)]
    o_stack = jnp.concatenate(onehot, axis=0).astype(jnp.bfloat16)
    cnt = jnp.dot(o_stack, upper, preferred_element_type=jnp.float32)

    iota_p = lax.broadcasted_iota(jnp.int32, (SLOTS, TB), 0)
    lane_f = lane_e.astype(jnp.float32)
    carry = jnp.zeros((N_EXP, 1), jnp.float32)
    bnd = jnp.zeros((N_EXP, TB), jnp.float32)
    a_parts, b_parts = [], []
    for b in range(N_TB):
        ob = onehot[b]
        if b % (N_TB // N_DEV) == 0:
            d = b // (N_TB // N_DEV)
            bnd = jnp.where(lane_e == BND0 + d, carry, bnd)
        cb = cnt[b * N_EXP:(b + 1) * N_EXP, :] + carry
        pos_b = jnp.sum(ob * cb, axis=0, keepdims=True).astype(jnp.int32)
        a_parts.append(jnp.concatenate([ob * lane_f, ob * float(b)], axis=0))
        b_parts.append(jnp.where(iota_p == pos_b, 1.0, 0.0))
        carry = carry + jnp.sum(ob, axis=1, keepdims=True)
    bnd = jnp.where(lane_e == BND0 + N_DEV, carry, bnd)
    bnd = jnp.minimum(bnd, float(CAP))
    a_mat = jnp.concatenate(a_parts, axis=1).astype(jnp.bfloat16)
    b_mat = jnp.concatenate(b_parts, axis=1).astype(jnp.bfloat16)
    t2 = lax.dot_general(a_mat, b_mat, (((1,), (1,)), ((), ())),
                         preferred_element_type=jnp.float32)
    tok = t2[:N_EXP, :] + float(TB) * t2[N_EXP:, :]
    tok = jnp.concatenate(
        [tok, jnp.zeros((N_EXP, TB - SLOTS), jnp.float32)], axis=1)
    tbl_v[...] = (tok + bnd).astype(jnp.int32)
    tbl_cp = pltpu.make_async_copy(tbl_v, tbl_s, tbl_sem)
    tbl_cp.start()

    out_ref[...] = jnp.zeros_like(out_ref)
    tbl_cp.wait()

    def gather(j):
        e = me * E_LOC + j
        for p in range(CAP):
            t = tbl_s[e, p]
            pltpu.make_async_copy(
                x_hbm.at[pl.ds(t, 1)], xg.at[pl.ds(j * SLOTS + p, 1)],
                g_sems.at[j]).start()

    with _scope("issue01"):
        gather(0)
        gather(1)
        w_copy(1).start()

    with _scope("barrier"):
        pl.semaphore_wait(barrier_sem, N_DEV - 1)

    def piece_copy(j, c_lo, nchunk, dst, ks):
        if nchunk == N_CHUNK:
            rows = pl.ds(0, ROWS)
        else:
            c0 = jnp.minimum(c_lo, N_CHUNK - nchunk)
            rows = pl.ds(pl.multiple_of(c0 * CHUNK, CHUNK), nchunk * CHUNK)
        return pltpu.make_async_remote_copy(
            src_ref=ysend.at[j, rows],
            dst_ref=stage.at[N_DEV - 1 - ks, j, rows],
            send_sem=send_sem,
            recv_sem=recv_sems.at[(N_DEV - 1 - ks) * E_LOC + j],
            device_id=(dst,), device_id_type=pl.DeviceIdType.MESH)

    def piece_op(j, e, d, dst, ks, op):
        lo = tbl_s[e, BND0 + d]
        hi = tbl_s[e, BND0 + d + 1]
        c_lo = lo >> 3
        need = ((hi + (CHUNK - 1)) >> 3) - c_lo
        sel = jnp.where(hi > lo, 1, 0)
        for n in PIECES[:-1]:
            sel = sel + jnp.where(need > n, 1, 0)
        branches = [lambda: None] + [
            (lambda n=n: op(piece_copy(j, c_lo, n, dst, ks))) for n in PIECES]
        lax.switch(sel, branches)
        return lo, hi

    def send(j, start):
        e = me * E_LOC + j
        for k in range(1, N_DEV):
            d = (me + k) % N_DEV
            piece_op(j, e, d, d, k,
                     (lambda c: c.start()) if start
                     else (lambda c: c.wait_send()))

    def copy_rows(buf, e, lo, hi):
        def rows(i, carry_):
            for u in range(UNROLL):
                p = jnp.minimum(lo + i * UNROLL + u, hi - 1)
                r = tbl_s[e, p] - me * TOK_PER_DEV
                wv = buf[pl.ds(p, 1), :]
                out_ref[pl.ds(r, 1), 0:HALF] = lax.bitcast_convert_type(
                    wv << 16, jnp.float32)
                out_ref[pl.ds(r, 1), HALF:D_OUT] = lax.bitcast_convert_type(
                    wv & jnp.uint32(0xFFFF0000), jnp.float32)
            return carry_

        lax.fori_loop(0, (hi - lo + (UNROLL - 1)) // UNROLL, rows, 0)

    def receive(j):
        for k in range(1, N_DEV):
            s = (me + k) % N_DEV
            e = s * E_LOC + j
            lo, hi = piece_op(j, e, me, me, N_DEV - k,
                              lambda c: c.wait_recv())
            copy_rows(stage.at[k - 1, j], e, lo, hi)

    def finish(j):
        with _scope("recv%d" % j):
            receive(j)
        with _scope("wsend%d" % j):
            send(j, False)

    for j in range(E_LOC):
        e = me * E_LOC + j
        with _scope("wait%d" % j):
            pltpu.make_async_copy(
                x_hbm.at[pl.ds(0, 48)], xg.at[pl.ds(j * SLOTS, 48)],
                g_sems.at[j]).wait()
            for p in range(48, CAP):
                pltpu.make_async_copy(
                    x_hbm.at[pl.ds(0, 1)], xg.at[pl.ds(j * SLOTS + p, 1)],
                    g_sems.at[j]).wait()
            w_copy(j).wait()
        with _scope("mm%d" % j):
            xb = xg[pl.ds(j * SLOTS, SLOTS), :].astype(jnp.bfloat16)
            wb = wbuf[j].astype(jnp.bfloat16)
            y = jnp.dot(xb, wb, preferred_element_type=jnp.float32)[:ROWS]
            yr = lax.bitcast_convert_type(
                y.astype(jnp.bfloat16).astype(jnp.float32), jnp.uint32)
            ysend[j] = yr[:, HALF:] | (yr[:, :HALF] >> 16)
        with _scope("send%d" % j):
            send(j, True)
        with _scope("own%d" % j):
            copy_rows(ysend.at[j], e, tbl_s[e, BND0 + me],
                      tbl_s[e, BND0 + me + 1])
        if j + 2 < E_LOC:
            with _scope("issue%d" % (j + 2)):
                gather(j + 2)
                w_copy(j + 2).start()
        if j >= 2:
            finish(j - 2)
    finish(E_LOC - 2)
    finish(E_LOC - 1)


def pallas_dist_moe_cap_ep_outshard_n2048_d512_e8_h1024_kernel(
    x: jax.Array,
    router_W: jax.Array,
    route_idx: jax.Array,
    expert_W: jax.Array,
):
    del router_W
    idx = route_idx.astype(jnp.int32).reshape(N_TB, TB)
    return pl.pallas_call(
        _kernel_body,
        out_shape=pltpu.VMEM((TOK_PER_DEV, D_OUT), jnp.float32),
        in_specs=[
            pl.BlockSpec(memory_space=pltpu.VMEM),
            pl.BlockSpec(memory_space=pl.ANY),
            pl.BlockSpec(memory_space=pl.ANY),
        ],
        out_specs=pl.BlockSpec(memory_space=pltpu.VMEM),
        scratch_shapes=[
            pltpu.VMEM((E_LOC, D_IN, D_OUT), jnp.float32),
            pltpu.VMEM((E_LOC * SLOTS, D_IN), jnp.float32),
            pltpu.VMEM((E_LOC, ROWS, HALF), jnp.uint32),
            pltpu.VMEM((N_DEV - 1, E_LOC, ROWS, HALF), jnp.uint32),
            pltpu.VMEM((N_EXP, TB), jnp.int32),
            pltpu.SMEM((N_EXP, TB), jnp.int32),
            pltpu.SemaphoreType.DMA((E_LOC,)),
            pltpu.SemaphoreType.DMA((E_LOC,)),
            pltpu.SemaphoreType.DMA,
            pltpu.SemaphoreType.DMA,
            pltpu.SemaphoreType.DMA(((N_DEV - 1) * E_LOC,)),
        ],
        compiler_params=pltpu.CompilerParams(
            collective_id=0,
            vmem_limit_bytes=64 * 1024 * 1024,
        ),
    )(idx, x, expert_W)
```

```python
import contextlib

import jax
import jax.numpy as jnp
from jax import lax
from jax.experimental import pallas as pl
from jax.experimental.pallas import tpu as pltpu

N_TOK = 2048
D_IN = 512
D_OUT = 1024
N_DEV = 4
E_LOC = 8
N_EXP = N_DEV * E_LOC
CAP = 51
SLOTS = 64
CHUNK = 8
N_CHUNK = 7
ROWS = N_CHUNK * CHUNK
PIECES = (2, 3, 4, N_CHUNK)
TOK_PER_DEV = N_TOK // N_DEV
TB = 128
N_TB = N_TOK // TB
HALF = D_OUT // 2
BND0 = SLOTS
UNROLL = 4
LAST = E_LOC - 1
QUART = D_OUT // 4

_PROFILE = False


def _scope(name):
    return jax.named_scope(name) if _PROFILE else contextlib.nullcontext()


def _kernel_body(idx_ref, x_hbm, w_hbm, out_ref,
                 wbuf, xg, ysend, stage, ysend_l, stage_l, tbl_v, tbl_s,
                 in_sems, tbl_sem, send_sem, recv_sems):
    me = lax.axis_index("i")

    def w_copy(j, h=None):
        if h is None:
            return pltpu.make_async_copy(
                w_hbm.at[j], wbuf.at[j], in_sems.at[j])
        cols = pl.ds(h * HALF, HALF)
        return pltpu.make_async_copy(
            w_hbm.at[j, :, cols], wbuf.at[j, :, cols], in_sems.at[j + h])

    w_copy(0).start()

    barrier_sem = pltpu.get_barrier_semaphore()
    for k in range(1, N_DEV):
        pl.semaphore_signal(
            barrier_sem, inc=1, device_id=((me + k) % N_DEV,),
            device_id_type=pl.DeviceIdType.MESH)

    eidx = idx_ref[...]
    iota_e = lax.broadcasted_iota(jnp.int32, (N_EXP, TB), 0)
    lane_e = lax.broadcasted_iota(jnp.int32, (N_EXP, TB), 1)
    sub_t = lax.broadcasted_iota(jnp.int32, (TB, TB), 0)
    lane_t = lax.broadcasted_iota(jnp.int32, (TB, TB), 1)
    upper = jnp.where(sub_t < lane_t, 1.0, 0.0).astype(jnp.bfloat16)
    onehot = [jnp.where(iota_e == eidx[b:b + 1, :], 1.0, 0.0)
              for b in range(N_TB)]
    o_stack = jnp.concatenate(onehot, axis=0).astype(jnp.bfloat16)
    cnt = jnp.dot(o_stack, upper, preferred_element_type=jnp.float32)

    iota_p = lax.broadcasted_iota(jnp.int32, (SLOTS, TB), 0)
    lane_f = lane_e.astype(jnp.float32)
    carry = jnp.zeros((N_EXP, 1), jnp.float32)
    bnd = jnp.zeros((N_EXP, TB), jnp.float32)
    a_parts, b_parts = [], []
    for b in range(N_TB):
        ob = onehot[b]
        if b % (N_TB // N_DEV) == 0:
            d = b // (N_TB // N_DEV)
            bnd = jnp.where(lane_e == BND0 + d, carry, bnd)
        cb = cnt[b * N_EXP:(b + 1) * N_EXP, :] + carry
        pos_b = jnp.sum(ob * cb, axis=0, keepdims=True).astype(jnp.int32)
        a_parts.append(jnp.concatenate([ob * lane_f, ob * float(b)], axis=0))
        b_parts.append(jnp.where(iota_p == pos_b, 1.0, 0.0))
        carry = carry + jnp.sum(ob, axis=1, keepdims=True)
    bnd = jnp.where(lane_e == BND0 + N_DEV, carry, bnd)
    bnd = jnp.minimum(bnd, float(CAP))
    a_mat = jnp.concatenate(a_parts, axis=1).astype(jnp.bfloat16)
    b_mat = jnp.concatenate(b_parts, axis=1).astype(jnp.bfloat16)
    t2 = lax.dot_general(a_mat, b_mat, (((1,), (1,)), ((), ())),
                         preferred_element_type=jnp.float32)
    tok = t2[:N_EXP, :] + float(TB) * t2[N_EXP:, :]
    tok = jnp.concatenate(
        [tok, jnp.zeros((N_EXP, TB - SLOTS), jnp.float32)], axis=1)
    tbl_v[...] = (tok + bnd).astype(jnp.int32)
    tbl_cp = pltpu.make_async_copy(tbl_v, tbl_s, tbl_sem)
    tbl_cp.start()

    out_ref[...] = jnp.zeros_like(out_ref)
    tbl_cp.wait()

    def gather(j):
        e = me * E_LOC + j
        for p in range(CAP):
            t = tbl_s[e, p]
            pltpu.make_async_copy(
                x_hbm.at[pl.ds(t, 1)], xg.at[pl.ds(j * SLOTS + p, 1)],
                in_sems.at[j]).start()

    with _scope("issue01"):
        gather(0)
        gather(1)
        w_copy(1).start()

    with _scope("barrier"):
        pl.semaphore_wait(barrier_sem, N_DEV - 1)

    def piece_copy(j, h, c_lo, nchunk, dst, ks):
        if nchunk == N_CHUNK:
            rows = pl.ds(0, ROWS)
        else:
            c0 = jnp.minimum(c_lo, N_CHUNK - nchunk)
            rows = pl.ds(pl.multiple_of(c0 * CHUNK, CHUNK), nchunk * CHUNK)
        slot = N_DEV - 1 - ks
        if h is None:
            src, dst_ref = ysend.at[j, rows], stage.at[slot, j, rows]
            sem = recv_sems.at[slot * (E_LOC + 1) + j]
        else:
            src, dst_ref = ysend_l.at[h, rows], stage_l.at[slot, h, rows]
            sem = recv_sems.at[slot * (E_LOC + 1) + j + h]
        return pltpu.make_async_remote_copy(
            src_ref=src, dst_ref=dst_ref, send_sem=send_sem, recv_sem=sem,
            device_id=(dst,), device_id_type=pl.DeviceIdType.MESH)

    def piece_op(j, hs, e, d, dst, ks, op):
        lo = tbl_s[e, BND0 + d]
        hi = tbl_s[e, BND0 + d + 1]
        c_lo = lo >> 3
        need = ((hi + (CHUNK - 1)) >> 3) - c_lo
        sel = jnp.where(hi > lo, 1, 0)
        for n in PIECES[:-1]:
            sel = sel + jnp.where(need > n, 1, 0)
        def branch(n):
            for h in hs:
                op(piece_copy(j, h, c_lo, n, dst, ks))

        branches = [lambda: None] + [
            (lambda n=n: branch(n)) for n in PIECES]
        lax.switch(sel, branches)
        return lo, hi

    def send(j, hs, start):
        e = me * E_LOC + j
        for k in (2, 1, 3):
            d = (me + k) % N_DEV
            piece_op(j, hs, e, d, d, k,
                     (lambda c: c.start()) if start
                     else (lambda c: c.wait_send()))

    def copy_rows(bufs, e, lo, hi):
        def rows(i, carry_):
            for u in range(UNROLL):
                p = jnp.minimum(lo + i * UNROLL + u, hi - 1)
                r = tbl_s[e, p] - me * TOK_PER_DEV
                c0 = 0
                for buf in bufs:
                    wv = buf[pl.ds(p, 1), :]
                    w = wv.shape[1]
                    out_ref[pl.ds(r, 1), c0:c0 + w] = (
                        lax.bitcast_convert_type(wv << 16, jnp.float32))
                    out_ref[pl.ds(r, 1), c0 + w:c0 + 2 * w] = (
                        lax.bitcast_convert_type(
                            wv & jnp.uint32(0xFFFF0000), jnp.float32))
                    c0 += 2 * w
            return carry_

        lax.fori_loop(0, (hi - lo + (UNROLL - 1)) // UNROLL, rows, 0)

    def halves(j):
        return (0, 1) if j == LAST else (None,)

    def receive(j):
        for k in (1, 3, 2):
            s = (me + k) % N_DEV
            e = s * E_LOC + j
            lo, hi = piece_op(j, halves(j), e, me, me, N_DEV - k,
                              lambda c: c.wait_recv())
            if j == LAST:
                bufs = [stage_l.at[k - 1, 0], stage_l.at[k - 1, 1]]
            else:
                bufs = [stage.at[k - 1, j]]
            copy_rows(bufs, e, lo, hi)

    def finish(j):
        with _scope("recv%d" % j):
            receive(j)
        with _scope("wsend%d" % j):
            send(j, halves(j), False)

    def pack(y):
        yr = lax.bitcast_convert_type(
            y[:ROWS].astype(jnp.bfloat16).astype(jnp.float32), jnp.uint32)
        w = yr.shape[1] // 2
        return yr[:, w:] | (yr[:, :w] >> 16)

    for j in range(E_LOC):
        e = me * E_LOC + j
        for h in halves(j):
            with _scope("wait%d" % j):
                if h is None or h == 0:
                    pltpu.make_async_copy(
                        x_hbm.at[pl.ds(0, 48)], xg.at[pl.ds(j * SLOTS, 48)],
                        in_sems.at[j]).wait()
                    for p in range(48, CAP):
                        pltpu.make_async_copy(
                            x_hbm.at[pl.ds(0, 1)],
                            xg.at[pl.ds(j * SLOTS + p, 1)],
                            in_sems.at[j]).wait()
                w_copy(j, h).wait()
            with _scope("mm%d" % j):
                xb = xg[pl.ds(j * SLOTS, SLOTS), :].astype(jnp.bfloat16)
                if h is None:
                    wb = wbuf[j].astype(jnp.bfloat16)
                else:
                    wb = wbuf[j, :, h * HALF:(h + 1) * HALF].astype(
                        jnp.bfloat16)
                y = jnp.dot(xb, wb, preferred_element_type=jnp.float32)
                if h is None:
                    ysend[j] = pack(y)
                else:
                    ysend_l[h] = pack(y)
            with _scope("send%d" % j):
                send(j, (h,), True)
            if h == 0:
                finish(j - 2)
        with _scope("own%d" % j):
            if j == LAST:
                bufs = [ysend_l.at[0], ysend_l.at[1]]
            else:
                bufs = [ysend.at[j]]
            copy_rows(bufs, e, tbl_s[e, BND0 + me], tbl_s[e, BND0 + me + 1])
        if j + 2 < E_LOC:
            with _scope("issue%d" % (j + 2)):
                gather(j + 2)
                for h in halves(j + 2):
                    w_copy(j + 2, h).start()
        if 2 <= j < LAST:
            finish(j - 2)
    finish(E_LOC - 2)
    finish(E_LOC - 1)


def pallas_dist_moe_cap_ep_outshard_n2048_d512_e8_h1024_kernel(
    x: jax.Array,
    router_W: jax.Array,
    route_idx: jax.Array,
    expert_W: jax.Array,
):
    del router_W
    idx = route_idx.astype(jnp.int32).reshape(N_TB, TB)
    return pl.pallas_call(
        _kernel_body,
        out_shape=pltpu.VMEM((TOK_PER_DEV, D_OUT), jnp.float32),
        in_specs=[
            pl.BlockSpec(memory_space=pltpu.VMEM),
            pl.BlockSpec(memory_space=pl.ANY),
            pl.BlockSpec(memory_space=pl.ANY),
        ],
        out_specs=pl.BlockSpec(memory_space=pltpu.VMEM),
        scratch_shapes=[
            pltpu.VMEM((E_LOC, D_IN, D_OUT), jnp.float32),
            pltpu.VMEM((E_LOC * SLOTS, D_IN), jnp.float32),
            pltpu.VMEM((LAST, ROWS, HALF), jnp.uint32),
            pltpu.VMEM((N_DEV - 1, LAST, ROWS, HALF), jnp.uint32),
            pltpu.VMEM((2, ROWS, QUART), jnp.uint32),
            pltpu.VMEM((N_DEV - 1, 2, ROWS, QUART), jnp.uint32),
            pltpu.VMEM((N_EXP, TB), jnp.int32),
            pltpu.SMEM((N_EXP, TB), jnp.int32),
            pltpu.SemaphoreType.DMA((E_LOC + 1,)),
            pltpu.SemaphoreType.DMA,
            pltpu.SemaphoreType.DMA,
            pltpu.SemaphoreType.DMA(((N_DEV - 1) * (E_LOC + 1),)),
        ],
        compiler_params=pltpu.CompilerParams(
            collective_id=0,
            vmem_limit_bytes=64 * 1024 * 1024,
        ),
    )(idx, x, expert_W)
```
